```python
import numpy as np

kernel_name = "dist_rmsnorm_colshard_i_m768_n512"

def setup_inputs():
    x = np.random.randn(768, 2048).astype(np.float32)
    gamma = np.random.randn(2048).astype(np.float32)
    return {"x": x, "gamma": gamma}

def reference(x: np.ndarray, gamma: np.ndarray) -> np.ndarray:
    eps = 1e-5
    rms = np.sqrt(np.mean(x * x, axis=1, keepdims=True) + eps)
    return gamma * x / rms
```

```python
import jax
import jax.numpy as jnp
from jax import lax
from jax.experimental import pallas as pl
from jax.experimental.pallas import tpu as pltpu

N_DEV = 4
EPS = 1e-5
LANES = 128
SUBLANES = 8
CHUNK_ROWS = (384, 192, 128, 64)
PEER_ORDER = (2, 1, 3)
OUT_DTYPE = jnp.bfloat16


def pallas_dist_rmsnorm_colshard_i_m768_n512_kernel(x: jax.Array, gamma: jax.Array):
    m, n = x.shape
    assert sum(CHUNK_ROWS) == m and n % LANES == 0
    n_chunks = len(CHUNK_ROWS)
    starts = [sum(CHUNK_ROWS[:i]) for i in range(n_chunks)]
    groups = [pl.cdiv(rows, LANES) for rows in CHUNK_ROWS]

    def body(x_hbm, g_hbm, o_ref, xv, gv, load_sems, g_sem, send_sem, recv_sems, *bufs):
        mine, theirs = bufs[:n_chunks], bufs[n_chunks:]
        loads = []
        for i in range(n_chunks):
            rows = pl.ds(starts[i], CHUNK_ROWS[i])
            loads.append(pltpu.make_async_copy(x_hbm.at[rows], xv.at[rows], load_sems.at[i]))
            loads[i].start()
        g_load = pltpu.make_async_copy(g_hbm, gv, g_sem)
        g_load.start()

        me = lax.axis_index("i")
        barrier = pltpu.get_barrier_semaphore()
        for k in PEER_ORDER:
            pl.semaphore_signal(barrier, 1, device_id=((me + k) % N_DEV,),
                                device_id_type=pl.DeviceIdType.MESH)

        tile = (SUBLANES, LANES)
        diag = lax.broadcasted_iota(jnp.int32, tile, 1) - lax.broadcasted_iota(jnp.int32, tile, 0)

        sends = []
        for i in range(n_chunks):
            loads[i].wait()
            for q in range(groups[i]):
                base = starts[i] + q * LANES
                acc = jnp.zeros(tile, jnp.float32)
                for r in range(0, min(LANES, CHUNK_ROWS[i] - q * LANES), SUBLANES):
                    v = xv[base + r:base + r + SUBLANES, :]
                    acc = jnp.where(diag == r, jnp.sum(v * v, axis=1, keepdims=True), acc)
                mine[i][:, q * LANES:(q + 1) * LANES] = jnp.sum(acc, axis=0, keepdims=True)
            if i == 0:
                pl.semaphore_wait(barrier, N_DEV - 1)
            for k in PEER_ORDER:
                sends.append(pltpu.make_async_remote_copy(
                    mine[i], theirs[i].at[k - 1], send_sem, recv_sems.at[i],
                    device_id=((me + k) % N_DEV,), device_id_type=pl.DeviceIdType.MESH))
                sends[-1].start()

        g_load.wait()
        g = jnp.broadcast_to(gv[...], (SUBLANES, n))
        for i in range(n_chunks):
            if i == n_chunks - 1:
                for send in sends:
                    send.wait_send()
            pltpu.make_async_copy(theirs[i], theirs[i], recv_sems.at[i]).wait()
            for q in range(groups[i]):
                base = starts[i] + q * LANES
                lanes = slice(q * LANES, (q + 1) * LANES)
                parts = [mine[i][:, lanes]] + [theirs[i][k, :, lanes] for k in range(N_DEV - 1)]
                parts = [jnp.broadcast_to(p, tile) for p in parts]
                total = (parts[0] + parts[1]) + (parts[2] + parts[3])
                inv = lax.rsqrt(total * (1.0 / (n * N_DEV)) + EPS)

                def scaled(r):
                    col = jnp.sum(jnp.where(diag == r, inv, 0.0), axis=1, keepdims=True)
                    return (xv[base + r:base + r + SUBLANES, :] * g) * col

                for r in range(0, min(LANES, CHUNK_ROWS[i] - q * LANES), 2 * SUBLANES):
                    y = jnp.concatenate([scaled(r), scaled(r + SUBLANES)], axis=0)
                    o_ref[base + r:base + r + 2 * SUBLANES, :] = y.astype(o_ref.dtype)

    return pl.pallas_call(
        body,
        out_shape=jax.ShapeDtypeStruct((m, n), OUT_DTYPE),
        in_specs=[pl.BlockSpec(memory_space=pltpu.HBM)] * 2,
        out_specs=pl.BlockSpec(memory_space=pltpu.VMEM),
        scratch_shapes=[
            pltpu.VMEM((m, n), jnp.float32),
            pltpu.VMEM((1, n), jnp.float32),
            pltpu.SemaphoreType.DMA((n_chunks,)),
            pltpu.SemaphoreType.DMA,
            pltpu.SemaphoreType.DMA,
            pltpu.SemaphoreType.DMA((n_chunks,)),
            *[pltpu.VMEM((1, q * LANES), jnp.float32) for q in groups],
            *[pltpu.VMEM((N_DEV - 1, 1, q * LANES), jnp.float32) for q in groups],
        ],
        compiler_params=pltpu.CompilerParams(
            collective_id=0, disable_bounds_checks=True, disable_semaphore_checks=True),
    )(x, gamma.reshape(1, n))
```

```python
import jax
import jax.numpy as jnp
from jax import lax
from jax.experimental import pallas as pl
from jax.experimental.pallas import tpu as pltpu

N_DEV = 4
EPS = 1e-5
SUBLANES, LANES = 8, 128
TILE = (SUBLANES, LANES)
STEP = 2 * SUBLANES
GROUP = 2 * LANES
CHUNK_ROWS = (384, 224, 112, 48)
FAR = 2
NEAR = (1, 3)
OUT_DTYPE = jnp.bfloat16


def _pack(lo, hi):
    def bits(v):
        return lax.bitcast_convert_type(v.astype(jnp.bfloat16).astype(jnp.float32), jnp.int32)

    return lax.shift_right_logical(bits(lo), 16) | bits(hi)


def _unpack(word):
    return (
        lax.bitcast_convert_type(word << 16, jnp.float32),
        lax.bitcast_convert_type(word & jnp.int32(-65536), jnp.float32),
    )


def _tree(fn, items):
    while len(items) > 1:
        items = [fn(a, b) for a, b in zip(items[::2], items[1::2])]
    return items[0]


def pallas_dist_rmsnorm_colshard_i_m768_n512_kernel(x: jax.Array, gamma: jax.Array):
    m, n = x.shape
    assert sum(CHUNK_ROWS) == m and all(rows % STEP == 0 for rows in CHUNK_ROWS)
    assert n == 4 * LANES
    n_chunks = len(CHUNK_ROWS)
    starts = [sum(CHUNK_ROWS[:i]) for i in range(n_chunks)]
    words = [pl.cdiv(rows, GROUP) * LANES for rows in CHUNK_ROWS]
    inv_count = 1.0 / (n * N_DEV)

    def groups(i):
        for r in range(0, CHUNK_ROWS[i], GROUP):
            yield starts[i] + r, min(GROUP, CHUNK_ROWS[i] - r), slice(r // 2, r // 2 + LANES)

    def body(x_hbm, g_hbm, o_ref, xv, gv, load_sems, send_sems, recv_sems, *bufs):
        mine, far, near_a, near_b = (
            bufs[k * n_chunks:(k + 1) * n_chunks] for k in range(N_DEV))

        loads = []
        for i in range(n_chunks):
            rows = pl.ds(starts[i], CHUNK_ROWS[i])
            loads.append(pltpu.make_async_copy(x_hbm.at[rows], xv.at[rows], load_sems.at[i]))
        g_load = pltpu.make_async_copy(g_hbm, gv, load_sems.at[n_chunks])
        for load in (*loads, g_load):
            load.start()

        me = lax.axis_index("i")

        def peer(distance):
            return dict(device_id=((me + distance) % N_DEV,),
                        device_id_type=pl.DeviceIdType.MESH)

        barrier = pltpu.get_barrier_semaphore()
        for distance in (FAR, *NEAR):
            pl.semaphore_signal(barrier, 1, **peer(distance))

        far_msgs, near_a_msgs, near_b_msgs = (
            [
                pltpu.make_async_remote_copy(
                    mine[i], dst[i],
                    send_sems.at[k * n_chunks + i], recv_sems.at[k * n_chunks + i],
                    **peer(distance))
                for i in range(n_chunks)
            ]
            for k, (dst, distance) in enumerate(zip((far, near_a, near_b), (FAR, *NEAR)))
        )

        sublane = lax.broadcasted_iota(jnp.int32, TILE, 0)
        diag = lax.broadcasted_iota(jnp.int32, TILE, 1) - sublane

        def sum_of_squares(row):
            v = xv[row:row + SUBLANES, :]
            v = v * v
            tiles = [v[:, c:c + LANES] for c in range(0, n, LANES)]
            return jnp.sum(_tree(jnp.add, tiles), axis=1, keepdims=True)

        for i in range(n_chunks):
            loads[i].wait()
            for row, count, lanes in groups(i):
                halves = [jnp.zeros(TILE, jnp.float32)] * 2
                for r in range(0, count, STEP):
                    halves = [
                        jnp.where(diag == r // 2, sum_of_squares(row + r + h * SUBLANES), halves[h])
                        for h in range(2)
                    ]
                mine[i][:, lanes] = jnp.sum(_pack(*halves), axis=0, keepdims=True)
            if i == 0:
                pl.semaphore_wait(barrier, N_DEV - 1)
            far_msgs[i].start()
            if i < n_chunks - 2:
                near_a_msgs[i].start()
                near_b_msgs[i].start()
        for i in range(n_chunks - 2, n_chunks):
            near_a_msgs[i].start()
            near_b_msgs[i].start()

        g_load.wait()
        g = jnp.broadcast_to(gv[...], (SUBLANES, n))
        for row in range(0, m, SUBLANES):
            xv[row:row + SUBLANES, :] = xv[row:row + SUBLANES, :] * g
        known = {}
        for i in range(n_chunks):
            near_a_msgs[i].wait_recv()
            near_b_msgs[i].wait_recv()
            for row, count, lanes in groups(i):
                parts = [_unpack(jnp.broadcast_to(buf[i][:, lanes], TILE))
                         for buf in (mine, near_a, near_b)]
                for h, (a, b, c) in enumerate(zip(*parts)):
                    partial = (a + b + c) * inv_count + EPS
                    for r in range(0, count, STEP):
                        known[row + r + h * SUBLANES] = jnp.sum(
                            jnp.where(diag == r // 2, partial, 0.0), axis=1, keepdims=True)
        for msg in (*far_msgs, *near_a_msgs, *near_b_msgs):
            msg.wait_send()

        for i in range(n_chunks):
            far_msgs[i].wait_recv()
            for r in range(0, CHUNK_ROWS[i], STEP):
                picks = [(s, jnp.full(TILE, far[i][0, r // 2 + s])) for s in range(SUBLANES)]
                _, word = _tree(
                    lambda a, b: (a[0], jnp.where(sublane < b[0], a[1], b[1])), picks)
                out = []
                for h, rest in enumerate(_unpack(word)):
                    row = starts[i] + r + h * SUBLANES
                    inv_rms = lax.rsqrt(rest * inv_count + known[row])
                    inv_rms = jnp.concatenate([inv_rms] * (n // LANES), axis=1)
                    out.append(xv[row:row + SUBLANES, :] * inv_rms)
                row = starts[i] + r
                o_ref[row:row + STEP, :] = jnp.concatenate(out, axis=0).astype(o_ref.dtype)

    n_msgs = (N_DEV - 1) * n_chunks
    return pl.pallas_call(
        body,
        out_shape=jax.ShapeDtypeStruct((m, n), OUT_DTYPE),
        in_specs=[pl.BlockSpec(memory_space=pltpu.HBM)] * 2,
        out_specs=pl.BlockSpec(memory_space=pltpu.VMEM),
        scratch_shapes=[
            pltpu.VMEM((m, n), jnp.float32),
            pltpu.VMEM((1, n), jnp.float32),
            pltpu.SemaphoreType.DMA((n_chunks + 1,)),
            pltpu.SemaphoreType.DMA((n_msgs,)),
            pltpu.SemaphoreType.DMA((n_msgs,)),
            *[space((1, w), jnp.int32)
              for space in (pltpu.VMEM, pltpu.SMEM, pltpu.VMEM, pltpu.VMEM) for w in words],
        ],
        compiler_params=pltpu.CompilerParams(collective_id=0, disable_semaphore_checks=True),
    )(x, gamma.reshape(1, n))
```

```python
import jax
import jax.numpy as jnp
from jax import lax
from jax.experimental import pallas as pl
from jax.experimental.pallas import tpu as pltpu

N_DEV = 4
EPS = 1e-5
SUBLANES, LANES = 8, 128
TILE = (SUBLANES, LANES)
STEP = 2 * SUBLANES
GROUP = 2 * LANES
HIGH_HALF = -(1 << 16)
CHUNK_ROWS = (416, 208, 96, 48)
FAR = 2
NEAR = (1, 3)
OUT_DTYPE = jnp.bfloat16


def _pack(lo, hi):
    def bits(v):
        return lax.bitcast_convert_type(v.astype(jnp.bfloat16).astype(jnp.float32), jnp.int32)

    return lax.shift_right_logical(bits(lo), 16) | (bits(hi) & HIGH_HALF)


def _unpack(word):
    return (
        lax.bitcast_convert_type(word << 16, jnp.float32),
        lax.bitcast_convert_type(word & HIGH_HALF, jnp.float32),
    )


def _tree(fn, items):
    while len(items) > 1:
        items = [fn(a, b) for a, b in zip(items[::2], items[1::2])]
    return items[0]


def pallas_dist_rmsnorm_colshard_i_m768_n512_kernel(x: jax.Array, gamma: jax.Array):
    m, n = x.shape
    assert sum(CHUNK_ROWS) == m and all(rows % STEP == 0 for rows in CHUNK_ROWS)
    assert n == 4 * LANES
    n_chunks = len(CHUNK_ROWS)
    starts = [sum(CHUNK_ROWS[:i]) for i in range(n_chunks)]
    words = [pl.cdiv(rows, GROUP) * LANES for rows in CHUNK_ROWS]
    inv_count = 1.0 / (n * N_DEV)

    def groups(i):
        for r in range(0, CHUNK_ROWS[i], GROUP):
            yield starts[i] + r, min(GROUP, CHUNK_ROWS[i] - r), slice(r // 2, r // 2 + LANES)

    def body(x_hbm, g_hbm, o_ref, xv, gv, load_sems, send_sems, recv_sems, *bufs):
        mine, far, near_a, near_b = (
            bufs[k * n_chunks:(k + 1) * n_chunks] for k in range(N_DEV))

        loads = []
        for i in range(n_chunks):
            rows = pl.ds(starts[i], CHUNK_ROWS[i])
            loads.append(pltpu.make_async_copy(x_hbm.at[rows], xv.at[rows], load_sems.at[i]))
        g_load = pltpu.make_async_copy(g_hbm, gv, load_sems.at[n_chunks])
        for load in (*loads, g_load):
            load.start()

        me = lax.axis_index("i")

        def peer(distance):
            return dict(device_id=((me + distance) % N_DEV,),
                        device_id_type=pl.DeviceIdType.MESH)

        barrier = pltpu.get_barrier_semaphore()
        for distance in (FAR, *NEAR):
            pl.semaphore_signal(barrier, 1, **peer(distance))

        far_msgs, near_a_msgs, near_b_msgs = (
            [
                pltpu.make_async_remote_copy(
                    mine[i], dst[i],
                    send_sems.at[k * n_chunks + i], recv_sems.at[k * n_chunks + i],
                    **peer(distance))
                for i in range(n_chunks)
            ]
            for k, (dst, distance) in enumerate(zip((far, near_a, near_b), (FAR, *NEAR)))
        )

        sublane = lax.broadcasted_iota(jnp.int32, TILE, 0)
        diag = lax.broadcasted_iota(jnp.int32, TILE, 1) - sublane

        def sum_of_squares(row):
            v = xv[row:row + SUBLANES, :]
            v = v * v
            tiles = [v[:, c:c + LANES] for c in range(0, n, LANES)]
            return jnp.sum(_tree(jnp.add, tiles), axis=1, keepdims=True)

        for i in range(n_chunks):
            loads[i].wait()
            for row, count, lanes in groups(i):
                halves = [jnp.zeros(TILE, jnp.float32)] * 2
                for r in range(0, count, STEP):
                    halves = [
                        jnp.where(diag == r // 2, sum_of_squares(row + r + h * SUBLANES), halves[h])
                        for h in range(2)
                    ]
                mine[i][:, lanes] = jnp.sum(_pack(*halves), axis=0, keepdims=True)
            if i == 0:
                pl.semaphore_wait(barrier, N_DEV - 1)
            far_msgs[i].start()
            if i < n_chunks - 2:
                near_a_msgs[i].start()
                near_b_msgs[i].start()
        for i in range(n_chunks - 2, n_chunks):
            near_a_msgs[i].start()
            near_b_msgs[i].start()

        g_load.wait()
        g = jnp.broadcast_to(gv[...], (SUBLANES, n))
        for row in range(0, m, SUBLANES):
            xv[row:row + SUBLANES, :] = xv[row:row + SUBLANES, :] * g
        known = {}
        for i in range(n_chunks):
            near_a_msgs[i].wait()
            near_b_msgs[i].wait()
            far_msgs[i].wait_send()
            for row, count, lanes in groups(i):
                parts = [_unpack(jnp.broadcast_to(buf[i][:, lanes], TILE))
                         for buf in (mine, near_a, near_b)]
                for h, (a, b, c) in enumerate(zip(*parts)):
                    partial = (a + b + c) * inv_count + EPS
                    for r in range(0, count, STEP):
                        known[row + r + h * SUBLANES] = jnp.sum(
                            jnp.where(diag == r // 2, partial, 0.0), axis=1, keepdims=True)

        for i in range(n_chunks):
            far_msgs[i].wait_recv()
            for r in range(0, CHUNK_ROWS[i], STEP):
                picks = [(s, jnp.full(TILE, far[i][0, r // 2 + s])) for s in range(SUBLANES)]
                _, word = _tree(
                    lambda a, b: (a[0], jnp.where(sublane < b[0], a[1], b[1])), picks)
                out = []
                for h, rest in enumerate(_unpack(word)):
                    row = starts[i] + r + h * SUBLANES
                    inv_rms = lax.rsqrt(rest * inv_count + known[row])
                    inv_rms = jnp.concatenate([inv_rms] * (n // LANES), axis=1)
                    out.append(xv[row:row + SUBLANES, :] * inv_rms)
                row = starts[i] + r
                o_ref[row:row + STEP, :] = jnp.concatenate(out, axis=0).astype(o_ref.dtype)

    n_msgs = (N_DEV - 1) * n_chunks
    return pl.pallas_call(
        body,
        out_shape=jax.ShapeDtypeStruct((m, n), OUT_DTYPE),
        in_specs=[pl.BlockSpec(memory_space=pltpu.HBM)] * 2,
        out_specs=pl.BlockSpec(memory_space=pltpu.VMEM),
        scratch_shapes=[
            pltpu.VMEM((m, n), jnp.float32),
            pltpu.VMEM((1, n), jnp.float32),
            pltpu.SemaphoreType.DMA((n_chunks + 1,)),
            pltpu.SemaphoreType.DMA((n_msgs,)),
            pltpu.SemaphoreType.DMA((n_msgs,)),
            *[space((1, w), jnp.int32)
              for space in (pltpu.VMEM, pltpu.SMEM, pltpu.VMEM, pltpu.VMEM) for w in words],
        ],
        compiler_params=pltpu.CompilerParams(collective_id=0, disable_semaphore_checks=True),
    )(x, gamma.reshape(1, n))
```
